```python
import numpy as np

kernel_name = "dist_rsx_agy_m2048_n1024"

def setup_inputs():
    return {"x": np.random.randn(2, 2048, 2048).astype(np.float32)}

def reference(x: np.ndarray) -> np.ndarray:
    return x.sum(axis=0)
```

```python
import jax
import jax.numpy as jnp
from jax import lax
from jax.experimental import pallas as pl
from jax.experimental.pallas import tpu as pltpu

_MESH = pl.DeviceIdType.MESH
_ROWS = 64
_AHEAD = 3


def pallas_dist_rsx_agy_m2048_n1024_kernel(x: jax.Array):
    _, m, n = x.shape
    chunks = m // _ROWS

    def body(x_hbm, o_ref, xf, sx, rx, ld_sem, sx_sem, rx_sem, sy_sem, ry_sem):
        mx = lax.axis_index("x")
        my = lax.axis_index("y")
        x_peer = (1 - mx, my)
        y_peer = (mx, 1 - my)
        cols = pl.ds(pl.multiple_of(my * n, n), n)

        def rows(k):
            return pl.ds(k * _ROWS, _ROWS)

        def load(k):
            return pltpu.make_async_copy(x_hbm.at[0, rows(k)], xf.at[rows(k)], ld_sem.at[k])

        def x_copy(k):
            return pltpu.make_async_remote_copy(
                sx.at[rows(k)], rx.at[rows(k)], sx_sem, rx_sem.at[k],
                device_id=x_peer, device_id_type=_MESH)

        def y_copy(r):
            return pltpu.make_async_remote_copy(
                o_ref.at[r, cols], o_ref.at[r, cols], sy_sem, ry_sem,
                device_id=y_peer, device_id_type=_MESH)

        for k in range(_AHEAD):
            load(k).start()
        barrier = pltpu.get_barrier_semaphore()
        for peer in (x_peer, y_peer):
            pl.semaphore_signal(barrier, 1, device_id=peer, device_id_type=_MESH)
        loaded = _AHEAD
        for k in range(chunks + _AHEAD):
            if k < chunks:
                load(k).wait()
                sx[rows(k), :] = xf[rows(k), :].astype(jnp.bfloat16)
                if k == 0:
                    pl.semaphore_wait(barrier, 2)
                x_copy(k).start()
                for _ in range(2):
                    if loaded < chunks:
                        load(loaded).start()
                        loaded += 1
            j = k - _AHEAD
            if j >= 0:
                x_copy(j).wait_recv()
                total = xf[rows(j), :] + rx[rows(j), :].astype(jnp.float32)
                o_ref[rows(j), cols] = total.astype(jnp.bfloat16)
                y_copy(rows(j)).start()

        pltpu.make_async_remote_copy(
            sx, rx, sx_sem, rx_sem.at[0], device_id=x_peer, device_id_type=_MESH).wait_send()
        y_copy(slice(None)).wait()

    return pl.pallas_call(
        body,
        out_shape=pltpu.VMEM((m, 2 * n), jnp.bfloat16),
        in_specs=[pl.BlockSpec(memory_space=pltpu.HBM)],
        out_specs=pl.BlockSpec(memory_space=pltpu.VMEM),
        scratch_shapes=[
            pltpu.VMEM((m, n), jnp.float32),
            pltpu.VMEM((m, n), jnp.bfloat16),
            pltpu.VMEM((m, n), jnp.bfloat16),
            pltpu.SemaphoreType.DMA((chunks,)),
            pltpu.SemaphoreType.DMA,
            pltpu.SemaphoreType.DMA((chunks,)),
            pltpu.SemaphoreType.DMA,
            pltpu.SemaphoreType.DMA,
        ],
        compiler_params=pltpu.CompilerParams(collective_id=0, vmem_limit_bytes=64 * 2**20),
    )(x)
```

```python
import jax
import jax.numpy as jnp
from jax import lax
from jax.experimental import pallas as pl
from jax.experimental.pallas import tpu as pltpu

LANES = 128
SLAB = 16
GROUP = 8
STREAM = 8
STREAM_MAX = STREAM + 1
PACKED = STREAM + 9 * (GROUP // 2)
FIRST = GROUP - 1
LAST = GROUP - 2
SHORT_STREAM = STREAM - 1
AHEAD = 2
BEHIND = 1


def _both(v):
    v = v << 16 | v
    return v - (1 << 32) if v >> 31 else v


def _shl(a, n):
    return lax.shift_left(a, jnp.int32(n) if isinstance(n, int) else n)


def _shr(a, n):
    return lax.shift_right_logical(a, jnp.int32(n) if isinstance(n, int) else n)


def _vregs(a, start, count=1):
    return a[:, start * LANES:(start + count) * LANES]


def _join(parts):
    return jnp.concatenate(parts, axis=1) if len(parts) > 1 else parts[0]


def _partner(a):
    return pltpu.roll(a, 4, 0)


def _reverse_bits(a):
    a = _shl(a, 16) | _shr(a, 16)
    for n, mask in ((8, 0x00FF), (4, 0x0F0F), (2, 0x3333), (1, 0x5555)):
        a = _shl(a & _both(mask), n) | (_shr(a, n) & _both(mask))
    return a


def _pick_key(words):
    count = words.shape[0] * words.shape[1]
    return (jnp.sum(_shr(words, 16) & 0x7FFF) >> (count.bit_length() - 1)) + 515


def _key_of_sum(a, b):
    return jnp.maximum(a, b) + jnp.maximum(64 - (jnp.abs(a - b) >> 1), 0)


def _offsets(words, key):
    return (key << 16 | key) - (words & _both(0x7FFF))


def _restore(high, low_plane, signs, key):
    low = _join([low_plane & _both(0xFF), _shr(low_plane, 8) & _both(0xFF)])
    for n in (1, 2, 4):
        signs = _join([signs, _shl(signs, n)])
    return ((key << 16 | key) - (high | low)) | (signs & _both(0x8000))


def _low_plane(t):
    t = t & _both(0xFF)
    return _vregs(t, 0, 4) | _shl(_vregs(t, 4, 4), 8)


def _high_plane(t):
    return _low_plane(_shr(t, 8))


def _from_high_plane(plane):
    return _join([_shl(plane, 8) & _both(0xFF00), plane & _both(0xFF00)])


def _signs(words):
    s = words & _both(0x8000)
    for n in (4, 2, 1):
        s = _vregs(s, 0, n) | _shr(_vregs(s, n, n), n)
    return s


def _live(runs):
    most = min(31 * runs, 32 * STREAM_MAX - 1 - 4 * (4 * GROUP - runs))
    return -(-most // 32)


def _push(stream, t, slabs_in):
    u = _shr(t, 8) & _both(31)
    n = u + (_shr(u + _both(28), 5) & _both(1)) + (_shr(_both(32) - u, 3) & _both(4))
    hi, lo = _shr(n, 16) & 31, n & 31
    hi0, lo0, hi1, lo1 = _vregs(hi, 0, 4), _vregs(lo, 0, 4), _vregs(hi, 4, 4), _vregs(lo, 4, 4)
    run = _shl(jnp.ones_like(lo0), lo0) | 1
    run = _shl(run, hi1) | 1
    run = _shl(run, lo1) | 1
    size = (hi0 + lo0) + (hi1 + lo1)
    bad = (_vregs(t, 0, 4) | _vregs(t, 4, 4)) & _both(0xE000)
    bad = bad | ((_vregs(n, 0, 4) | _vregs(n, 4, 4) | size) & _both(0xE0))
    bad = _vregs(bad, 0, 2) | _vregs(bad, 2, 2)
    size = jnp.minimum(size, 31)
    rest = 32 - size
    run = _shl(run, rest)
    for j in range(4):
        had, has = _live(4 * slabs_in + j), _live(4 * slabs_in + j + 1)
        carried = [_vregs(run, j)]
        if has > 1:
            carried.append(_shl(_vregs(stream, 0, has - 1), _join([_vregs(rest, j)] * (has - 1))))
        carried = _join(carried)
        if had:
            kept = _shr(stream, _join([_vregs(size, j)] * had)) | _vregs(carried, 0, had)
            carried = _join([kept, _vregs(carried, had)]) if has > had else kept
        stream = carried
    size = _vregs(size, 0, 2) + _vregs(size, 2, 2)
    return stream, _vregs(size, 0) + _vregs(size, 1), _vregs(bad, 0) | _vregs(bad, 1)


def _seal(stream, bits, bad, key, count):
    lane = lax.broadcasted_iota(jnp.int32, bits.shape, 1)
    sublane = lax.broadcasted_iota(jnp.int32, bits.shape, 0)
    bits = jnp.where((bad != 0) | (bits >= 32 * (count + 1)), 1 << 16, bits + 1)
    flag = jnp.where(bits + _partner(bits) > 64 * count, 1, 0)
    head = _shl(jnp.where(sublane < 4, _shr(jnp.broadcast_to(key, bits.shape), lane & 15), flag), 31)
    sent = _shr(_vregs(stream, 0, count + 1), 1) | _join([head, _shl(_vregs(stream, 0, count), 31)])
    last = _vregs(sent, count - 1) | _reverse_bits(_partner(_vregs(sent, count)))
    sent = _join([_vregs(sent, 0, count - 1), last])
    ones = _join([head | 0x7FFFFFFF] + [jnp.full_like(head, -1)] * (count - 1))
    return jnp.where(_join([flag] * count) != 0, ones, sent), flag


def _unseal(sent):
    count = sent.shape[1] // LANES
    head = _shr(_vregs(sent, 0), 31)
    lane = lax.broadcasted_iota(jnp.int32, head.shape, 1)
    sublane = lax.broadcasted_iota(jnp.int32, head.shape, 0)
    key_bit = jnp.where((lane < 16) & (sublane == 0), _shl(head, lane & 15), 0)
    header = jnp.sum(jnp.where(sublane < 4, key_bit, _shl(head, 16)))
    stream = _join([sent, _reverse_bits(_partner(_vregs(sent, count - 1)))])
    below = _join([_shr(_vregs(stream, 1, count), 31), jnp.zeros_like(head)])
    return _shl(stream, 1) | below, header & 0xFFFF, header >> 16


def _pop(stream, slabs_in):
    first, second = [None] * 4, [None] * 4
    for j in reversed(range(4)):
        window, zeros = _vregs(stream, 0), []
        for i in range(4):
            zeros.append(lax.clz(window))
            if i < 3:
                window = _shl(_shl(window, 1), zeros[i])
        first[j] = _shl(zeros[0], 24) | _shl(zeros[1], 8)
        second[j] = _shl(zeros[2], 24) | _shl(zeros[3], 8)
        had, has = _live(4 * (slabs_in - 1) + j + 1), _live(4 * (slabs_in - 1) + j)
        if has:
            most = (zeros[0] + zeros[1]) + (zeros[2] + 4)
            size, rest = most + zeros[3], (32 - most) - zeros[3]
            kept = _shl(_vregs(stream, 0, has), _join([size] * has))
            below = _shr(_vregs(stream, 1, had - 1), _join([rest] * (had - 1)))
            upper = _vregs(kept, 0, had - 1) | below
            stream = _join([upper, _vregs(kept, had - 1)]) if has == had else upper
    zeros = _join(first + second)
    at_least_4 = (zeros + _both(0x1C00)) & _both(0x2000)
    at_least_3 = (zeros + _both(0x1D00)) & _both(0x2000)
    return zeros + _both(0x0100) - _shr(at_least_3 ^ at_least_4, 3) - _shr(at_least_4, 5), stream


def _at(start, count=1):
    return pl.ds(start * LANES, count * LANES)


def _low_at(i):
    return _at(STREAM + 9 * (i // 2) + 5 * (i % 2), 4)


def _signs_at(i):
    return _at(STREAM + 9 * (i // 2) + 4)


def _rows(group, slab, count=1):
    start = (group * GROUP + slab) * SLAB
    return pl.ds(start if isinstance(start, int) else pl.multiple_of(start, SLAB), count * SLAB)


def _unless_head(group, slab, fn):
    if slab < FIRST:
        fn()
    else:
        pl.when(group > 0)(fn)


_X_KEY, _X_PLAIN, _SUM_KEY, _Y_KEY, _Y_PLAIN, _X_EXTRAS, _Y_EXTRAS = range(7)


def _body(x_hbm, out, local, tail, x_send, x_recv, y_send, y_recv, x_send_extra, x_recv_extra,
          y_send_extra, y_recv_extra, ends, pack_x, unpack_x, pack_y, unpack_y, x_high, y_high,
          keys, scalars, load_sems, send_sems, x_sems, y_sems, x_extra_sems, y_extra_sems,
          end_send_sems, end_recv_sems):
    groups = x_send.shape[0]
    width = local.shape[1]
    my_x, my_y = lax.axis_index("x"), lax.axis_index("y")
    x_peer, y_peer = (1 - my_x, my_y), (my_x, 1 - my_y)
    mine = pl.ds(pl.multiple_of(my_y * width, width), width)
    theirs = pl.ds(pl.multiple_of((1 - my_y) * width, width), width)


    def load(rows, slot):
        return pltpu.make_async_copy(x_hbm.at[0, rows], local.at[rows], load_sems.at[slot])

    def load_group(g):
        return load(_rows(g, 0, GROUP), GROUP - 1 + g)

    def remote(src, dst, send_sem, recv_sem, peer):
        return pltpu.make_async_remote_copy(
            src, dst, send_sem, recv_sem, device_id=peer, device_id_type=pl.DeviceIdType.MESH)

    def x_copy(g, slot, part):
        send_sem = send_sems.at[jnp.minimum(g, 1)]
        return remote(x_send.at[g, :, part], x_recv.at[g, :, part], send_sem,
                      x_sems.at[g * (GROUP + 1) + slot], x_peer)

    def x_stream(g, count=STREAM):
        return x_copy(g, GROUP, _at(0, count))

    def x_slab(g, i):
        return x_copy(g, i, _at(STREAM + 9 * (i // 2) + 5 * (i % 2), 5 - i % 2))

    def y_copy(g, slot, part):
        send_sem = send_sems.at[2 + jnp.minimum(g, 1) + g // (groups - 1)]
        return remote(y_send.at[g, :, part], y_recv.at[g, :, part], send_sem,
                      y_sems.at[2 * g + slot], y_peer)

    def y_slab(g, i, slot=0):
        return y_copy(g, slot, _at(STREAM + 9 * (i // 2) + 4 * (i % 2), 4 + i % 2))

    def x_extra(g):
        return remote(x_send_extra.at[g], x_recv_extra.at[g], send_sems.at[5], x_extra_sems.at[g], x_peer)

    def y_extra(g):
        return remote(y_send_extra.at[g], y_recv_extra.at[g], send_sems.at[6], y_extra_sems.at[g], y_peer)

    head_rows, tail_rows = _rows(0, FIRST), _rows(groups - 1, LAST, GROUP - LAST)
    head = pl.ds(0, SLAB)
    load_tail = pltpu.make_async_copy(x_hbm.at[0, tail_rows], tail, load_sems.at[GROUP + groups - 1])

    def end_copy(slot, src, dst, peer):
        return remote(src, dst, end_send_sems.at[slot], end_recv_sems.at[slot], peer)

    head_x = end_copy(0, ends.at[0, head], ends.at[1, head], x_peer)
    head_y = end_copy(1, out.at[head_rows, mine], out.at[head_rows, mine], y_peer)
    tail_y = end_copy(2, ends.at[2], ends.at[3], y_peer)
    tail_x = end_copy(3, ends.at[3], ends.at[4], x_peer)


    def push(saved, t, slabs_in):
        stream = saved[:, _at(0, _live(4 * slabs_in))] if slabs_in else None
        stream, bits, bad = _push(stream, t, slabs_in)
        if slabs_in:
            bits, bad = bits + saved[:, _at(STREAM_MAX)], bad | saved[:, _at(STREAM_MAX + 1)]
        if slabs_in < GROUP - 1:
            saved[:, _at(0, _live(4 * slabs_in + 4))] = stream
            saved[:, _at(STREAM_MAX, 2)] = _join([bits, bad])
        return stream, bits, bad

    def pop(saved, slabs_in, stream=None):
        if stream is None:
            stream = saved[:, _at(0, _live(4 * slabs_in))]
        high, stream = _pop(stream, slabs_in)
        if slabs_in > 1:
            saved[:, _at(0, _live(4 * slabs_in - 4))] = stream
        return high

    def signs_of(buf, g, i):
        signs = buf[g, :, _signs_at(i)]
        return _shl(signs, 8) if i % 2 else signs


    def local_words(g, i):
        return pltpu.bitcast(local[_rows(g, i), :].astype(jnp.bfloat16), jnp.int32)

    def pack_planes(g, i, words, key, first_of_pair):
        t = _offsets(words, key)
        x_send[g, :, _low_at(i)] = _low_plane(t)
        signs = _shr(_signs(words), 8) if i % 2 else _signs(words)
        x_send[g, :, _signs_at(i)] = signs if first_of_pair else signs | x_send[g, :, _signs_at(i)]
        return t

    def send_x_extra(g, flag, slabs):
        @pl.when(jnp.sum(flag) != 0)
        def _():
            scalars[_X_EXTRAS] = scalars[_X_EXTRAS] + 1

            @pl.loop(0, slabs)
            def _(i):
                x_send_extra[g, i] = _high_plane(_offsets(local_words(g, i), keys[g]))

            x_extra(g).start()

    def pack_first_group():
        stream = jnp.zeros((8, _live(4) * LANES), jnp.int32)
        bits = bad = jnp.zeros((8, LANES), jnp.int32)
        for i in reversed(range(FIRST)):
            load(_rows(0, i), i).wait()
            words = local_words(0, i)
            if i == FIRST - 1:
                key = _pick_key(words)
                keys[0] = key
            t = pack_planes(0, i, words, key, i % 2 or i == FIRST - 1)
            stream, more_bits, more_bad = _push(stream, t, GROUP - 1 - i)
            bits, bad = bits + more_bits, bad | more_bad
        x_send[0, :, _at(0, SHORT_STREAM)], flag = _seal(stream, bits, bad, key, SHORT_STREAM)
        x_stream(0, SHORT_STREAM).start()
        for i in range(FIRST):
            x_slab(0, i).start()
        load_tail.wait()
        ends[2] = tail[...].astype(jnp.bfloat16)
        tail_y.start()
        send_x_extra(0, flag, FIRST)

    def pack_step(g, step):
        i = GROUP - 1 - step
        if step == 0:
            load_group(g).wait()
            pl.when(g + 1 < groups)(lambda: load_group(jnp.minimum(g + 1, groups - 1)).start())
            words = local_words(g, i)
            key = _pick_key(words)
            keys[g] = key
        else:
            words, key = local_words(g, i), keys[g]
        stream, bits, bad = push(pack_x, pack_planes(g, i, words, key, i % 2), step)
        if i == 0:
            x_send[g, :, _at(0, STREAM)], pack_x[:, _at(0)] = _seal(stream, bits, bad, key, STREAM)
            x_stream(g).start()

    def send_slabs(g):
        send_x_extra(g, pack_x[:, _at(0)], GROUP)
        for i in range(GROUP):
            x_slab(g, i).start()


    def reduce_begin(g):
        @pl.when(g == 0)
        def _():
            x_stream(g, SHORT_STREAM).wait_recv()
            x_recv[g, :, _at(SHORT_STREAM)] = _reverse_bits(_partner(x_recv[g, :, _at(SHORT_STREAM - 1)]))

        pl.when(g > 0)(lambda: x_stream(g).wait_recv())
        stream, key, plain = _unseal(x_recv[g, :, _at(0, STREAM)])
        x_high[...] = pop(unpack_x, GROUP, stream)
        scalars[_X_KEY], scalars[_X_PLAIN] = key, plain
        scalars[_SUM_KEY] = _key_of_sum(key, keys[g])
        pl.when(plain != 0)(lambda: x_extra(g).wait_recv())

    def reduce_step(g, i):
        def arrive():
            @pl.when(scalars[_X_PLAIN] != 0)
            def _():
                x_high[...] = _from_high_plane(x_recv_extra[g, i])

            x_slab(g, i).wait_recv()

        _unless_head(g, i, arrive)
        got = _restore(x_high[...], x_recv[g, :, _low_at(i)], signs_of(x_recv, g, i), scalars[_X_KEY])
        total = local[_rows(g, i), :] + pltpu.bitcast(got, jnp.bfloat16).astype(jnp.float32)
        total = total.astype(jnp.bfloat16)

        def keep():
            out[_rows(g, i), mine] = total

        _unless_head(g, i, keep)
        if i < LAST:
            send_sum(g, i, pltpu.bitcast(total, jnp.int32))
        else:
            pl.when(g < groups - 1)(lambda: send_sum(g, i, pltpu.bitcast(total, jnp.int32)))
            if i < GROUP - 1:
                _unless_head(g, i + 1, lambda: pop_x(i + 1))

    def pop_x(i):
        x_high[...] = pop(unpack_x, GROUP - i)

    def send_sum(g, i, words):
        key = scalars[_SUM_KEY]
        t = _offsets(words, key)
        y_send[g, :, _low_at(i)] = _low_plane(t)
        signs = _signs(words)
        y_send[g, :, _signs_at(i)] = _shr(signs, 8) | y_send[g, :, _signs_at(i)] if i % 2 else signs
        if i == GROUP - 1:
            send_stream(g, push(pack_y, t, i), key, STREAM)
            return
        if i == LAST - 1:
            pl.when(g < groups - 1)(lambda: y_slab(g, i).start())
        else:
            y_slab(g, i).start()
        state = push(pack_y, t, i)
        if i < LAST:
            pop_x(i + 1)
        if i == LAST - 1:
            pl.when(g == groups - 1)(lambda: send_stream(g, state, key, SHORT_STREAM))

    def send_stream(g, state, key, count):
        part = _at(STREAM - count, count)
        y_send[g, :, part], flag = _seal(*state, key, count)
        y_copy(g, 0, part).start()
        if count == STREAM:
            pl.when(g > 0)(lambda: y_slab(g, GROUP - 1, 1).start())
            pl.when(g == 0)(lambda: y_copy(g, 0, _signs_at(FIRST)).start())
            slabs = jnp.where(g > 0, GROUP, FIRST)
        else:
            y_slab(g, LAST - 1, 1).start()
            slabs = LAST

        @pl.when(jnp.sum(flag) != 0)
        def _():
            scalars[_Y_EXTRAS] = scalars[_Y_EXTRAS] + 1

            @pl.loop(0, slabs)
            def _(j):
                sums = pltpu.bitcast(out[_rows(g, j), mine], jnp.int32)
                y_send_extra[g, j] = _high_plane(_offsets(sums, key))

            y_extra(g).start()


    def gather_slab(g, i, high, key):
        got = _restore(high, y_recv[g, :, _low_at(i)], signs_of(y_recv, g, i), key)
        out[_rows(g, i), theirs] = pltpu.bitcast(got, jnp.bfloat16)

    def gather_plain(g, slabs, key, plain):
        @pl.when(plain != 0)
        def _():
            y_extra(g).wait_recv()
            for i in range(slabs):
                _unless_head(g, i, lambda: gather_slab(g, i, _from_high_plane(y_recv_extra[g, i]), key))

    def gather_begin(g):
        pl.when(g == 0)(lambda: y_copy(g, 0, _at(0, PACKED - 4)).wait_recv())

        @pl.when(g > 0)
        def _():
            y_copy(g, 0, _at(0, PACKED - 5)).wait_recv()
            y_slab(g, GROUP - 1, 1).wait_recv()

        stream, scalars[_Y_KEY], scalars[_Y_PLAIN] = _unseal(y_recv[g, :, _at(0, STREAM)])
        y_high[...] = pop(unpack_y, GROUP, stream)

    def gather_step(g, step):
        i = GROUP - 1 - step
        high = y_high[...]
        if i > 0:
            y_high[...] = pop(unpack_y, i)
        _unless_head(g, i, lambda: gather_slab(g, i, high, scalars[_Y_KEY]))
        if i == 0:
            gather_plain(g, GROUP, scalars[_Y_KEY], scalars[_Y_PLAIN])

    def gather_last_group():
        g = groups - 1
        skip = STREAM - SHORT_STREAM
        y_copy(g, 0, _at(skip, SHORT_STREAM + 9 * (LAST // 2) - 5)).wait_recv()
        stream, key, plain = _unseal(y_recv[g, :, _at(skip, SHORT_STREAM)])
        high = [None] * LAST
        for i in reversed(range(LAST)):
            high[i], stream = _pop(stream, i + 1)
            if i < LAST - 2:
                gather_slab(g, i, high[i], key)
        y_slab(g, LAST - 1, 1).wait_recv()
        for i in (LAST - 2, LAST - 1):
            gather_slab(g, i, high[i], key)
        gather_plain(g, LAST, key, plain)


    load(head_rows, GROUP - 1).start()
    barrier = pltpu.get_barrier_semaphore()
    for peer in (x_peer, y_peer):
        pl.semaphore_signal(barrier, 1, device_id=peer, device_id_type=pl.DeviceIdType.MESH)
    for i in reversed(range(FIRST)):
        load(_rows(0, i), i).start()
    load_tail.start()
    load_group(1).start()
    scalars[_X_EXTRAS] = scalars[_Y_EXTRAS] = 0
    x_recv[0, :, _low_at(FIRST)] = jnp.zeros((8, 4 * LANES), jnp.int32)

    load(head_rows, GROUP - 1).wait()
    ends[0, head] = local[head_rows, :].astype(jnp.bfloat16)
    pl.semaphore_wait(barrier, 2)
    head_x.start()
    pack_first_group()

    @pl.loop(1, groups + AHEAD + BEHIND - 1)
    def _(k):
        def when_at(lag, fn, *args):
            g = k - lag
            pl.when(jnp.logical_and(g >= 0, g < groups))(lambda: fn(jnp.clip(g, 0, groups - 1), *args))

        def pack(*steps):
            for step in steps:
                when_at(0, pack_step, step)

        def reduce(i):
            when_at(AHEAD, reduce_step, i)

        def gather(*steps):
            for step in steps:
                when_at(AHEAD + BEHIND, gather_step, step)

        @pl.when(k == AHEAD)
        def _():
            head_x.wait_recv()
            total = local[head_rows, :] + ends[1, head].astype(jnp.float32)
            out[head_rows, mine] = total.astype(jnp.bfloat16)
            head_y.start()

        @pl.when(k == groups)
        def _():
            tail_y.wait_recv()
            tail_x.start()

        when_at(AHEAD, reduce_begin)
        reduce(0)
        pack(0)
        reduce(1)
        pack(1, 2, 3)
        reduce(2)
        pack(4, 5)
        reduce(3)
        pack(6, 7)
        reduce(4)
        when_at(0, send_slabs)
        reduce(5)
        when_at(AHEAD + BEHIND, gather_begin)
        gather(0)
        reduce(6)
        gather(1, 2)
        reduce(7)
        gather(3, 4, 5, 6, 7)

    head_y.wait_recv()
    for copy in (head_x, head_y, tail_y):
        copy.wait_send()
    x_copy(0, 0, _at(0, PACKED - 4 - (STREAM - SHORT_STREAM))).wait_send()
    y_copy(0, 0, _at(0, PACKED - 4)).wait_send()
    later, middle = pl.ds(1, groups - 1), pl.ds(1, groups - 2)
    remote(x_send.at[later], x_recv.at[later], send_sems.at[1], x_sems.at[0], x_peer).wait_send()
    remote(y_send.at[middle], y_recv.at[middle], send_sems.at[3], y_sems.at[0], y_peer).wait_send()
    pl.loop(0, scalars[_X_EXTRAS])(lambda _: x_extra(0).wait_send())

    gather_last_group()

    tail_x.wait()
    total = ends[3].astype(jnp.float32) + ends[4].astype(jnp.float32)
    out[tail_rows, theirs] = total.astype(jnp.bfloat16)
    y_copy(groups - 1, 0, _at(0, SHORT_STREAM + 9 * (LAST // 2))).wait_send()
    pl.loop(0, scalars[_Y_EXTRAS])(lambda _: y_extra(0).wait_send())


def pallas_dist_rsx_agy_m2048_n1024_kernel(x: jax.Array):
    _, rows, width = x.shape
    groups = rows // (GROUP * SLAB)
    assert width == 8 * LANES and rows == groups * GROUP * SLAB and groups > AHEAD
    packed = pltpu.VMEM((groups, 8, PACKED * LANES), jnp.int32)
    extra = pltpu.VMEM((groups, GROUP, 8, 4 * LANES), jnp.int32)
    packing = pltpu.VMEM((8, (STREAM_MAX + 2) * LANES), jnp.int32)
    unpacking = pltpu.VMEM((8, STREAM_MAX * LANES), jnp.int32)
    dma = pltpu.SemaphoreType.DMA
    return pl.pallas_call(
        _body,
        out_shape=pltpu.VMEM((rows, 2 * width), jnp.bfloat16),
        in_specs=[pl.BlockSpec(memory_space=pltpu.HBM)],
        out_specs=pl.BlockSpec(memory_space=pltpu.VMEM),
        scratch_shapes=[
            pltpu.VMEM((rows, width), jnp.float32),
            pltpu.VMEM(((GROUP - LAST) * SLAB, width), jnp.float32),
            packed, packed, packed, packed,
            extra, extra, extra, extra,
            pltpu.VMEM((5, (GROUP - LAST) * SLAB, width), jnp.bfloat16),
            packing, unpacking, packing, unpacking,
            pltpu.VMEM((8, width), jnp.int32),
            pltpu.VMEM((8, width), jnp.int32),
            pltpu.SMEM((groups,), jnp.int32),
            pltpu.SMEM((8,), jnp.int32),
            dma((GROUP + groups,)),
            dma((7,)),
            dma((groups * (GROUP + 1),)),
            dma((2 * groups,)),
            dma((groups,)),
            dma((groups,)),
            dma((4,)),
            dma((4,)),
        ],
        compiler_params=pltpu.CompilerParams(
            collective_id=0,
            vmem_limit_bytes=64 * 2**20,
            disable_semaphore_checks=True,
        ),
    )(x)
```
